```python
import numpy as np

kernel_name = "dist_ring_attn_i_s256_d64"

def setup_inputs():
    S, D = 1024, 64
    q = np.random.randn(S, D).astype(np.float32)
    k = np.random.randn(S, D).astype(np.float32)
    v = np.random.randn(S, D).astype(np.float32)
    return {"q": q, "k": k, "v": v}

def reference(q: np.ndarray, k: np.ndarray, v: np.ndarray) -> np.ndarray:
    D = q.shape[1]
    scores = q @ k.T / np.sqrt(D)
    scores_max = np.max(scores, axis=1, keepdims=True)
    weights = np.exp(scores - scores_max)
    weights = weights / np.sum(weights, axis=1, keepdims=True)
    return weights @ v
```

```python
import jax
import jax.numpy as jnp
from jax import lax
from jax.experimental import pallas as pl
from jax.experimental.pallas import tpu as pltpu

N_DEV = 4
N_CHUNK = 4
N_LOAD = 4
LOG2E = 1.4426950408889634
MESH = pl.DeviceIdType.MESH
CONTRACT_ROWS = (((0,), (0,)), ((), ()))
K_SEL, V_SEL = 0, 1
OWN, FROM_LEFT, DIAG, FROM_RIGHT = 0, 1, 2, 3


def pallas_dist_ring_attn_i_s256_d64_kernel(
    q: jax.Array,
    k: jax.Array,
    v: jax.Array,
):
    S, D = q.shape
    H = S // 2
    rows_c = D // N_CHUNK
    rows_l = D // N_LOAD
    group = N_CHUNK // N_LOAD
    scale = float(D) ** -0.5 * LOG2E

    def body(q_hbm, k_hbm, v_hbm, o_ref,
             f32buf, kbuf, vbuf, ld_sems, send_sems, recv_sems, go_sem):
        my = lax.axis_index("i")
        right = lax.rem(my + 1, N_DEV)
        left = lax.rem(my + N_DEV - 1, N_DEV)
        bufs = (kbuf, vbuf)

        def load(src, j, c):
            rows = pl.ds(c * rows_l, rows_l)
            return pltpu.make_async_copy(
                src.at[rows], f32buf.at[1 + j, rows], ld_sems.at[1 + j * N_LOAD + c])

        ld_k = [load(k_hbm, K_SEL, c) for c in range(N_LOAD)]
        ld_v = [load(v_hbm, V_SEL, c) for c in range(N_LOAD)]
        ld_q = pltpu.make_async_copy(q_hbm, f32buf.at[0], ld_sems.at[0])
        for c in ld_k + ld_v + [ld_q]:
            c.start()

        def signal(sem, target):
            pl.semaphore_signal(sem, inc=1, device_id=(target,), device_id_type=MESH)

        barrier = pltpu.get_barrier_semaphore()

        @pl.when(my != 2)
        def _():
            signal(barrier, left)
            signal(barrier, right)

        def rdma(sel, src, dst, half, kind, target, chunk=None):
            rows = pl.ds(0, D) if chunk is None else pl.ds(chunk * rows_c, rows_c)
            i = sel * N_CHUNK + (chunk or 0)
            return pltpu.make_async_remote_copy(
                src_ref=bufs[sel].at[src, half, rows],
                dst_ref=bufs[sel].at[dst, half, rows],
                send_sem=send_sems.at[kind, half, i],
                recv_sem=recv_sems.at[dst - 1, half, i],
                device_id=(target,), device_id_type=MESH)

        def chunked(sel, src, dst, half, kind, target):
            return [rdma(sel, src, dst, half, kind, target, c) for c in range(N_CHUNK)]

        lead_r = [chunked(s, OWN, FROM_LEFT, 0, 0, right) for s in (K_SEL, V_SEL)]
        lead_l = [chunked(s, OWN, FROM_RIGHT, 1, 1, left) for s in (K_SEL, V_SEL)]
        trail_r = [rdma(s, OWN, FROM_LEFT, 1, 0, right) for s in (K_SEL, V_SEL)]
        trail_l = [rdma(s, OWN, FROM_RIGHT, 0, 1, left) for s in (K_SEL, V_SEL)]
        fwd_r = [chunked(s, FROM_LEFT, DIAG, 0, 2, right) for s in (K_SEL, V_SEL)]
        fwd_l = [chunked(s, FROM_RIGHT, DIAG, 1, 3, left) for s in (K_SEL, V_SEL)]

        def start(copies):
            for c in copies:
                c.start()

        def start_both_sides(to_right, to_left):
            @pl.when((my == 0) | (my == 2))
            def _():
                start([c for pair in zip(to_right, to_left) for c in pair])

            @pl.when(my == 1)
            def _():
                start(to_left)

            @pl.when(my == 3)
            def _():
                start(to_right)

        def cast_and_send(sel, c):
            rows = slice(c * rows_l, (c + 1) * rows_l)
            for h in range(2):
                bufs[sel][OWN, h, rows] = f32buf[
                    1 + sel, rows, h * H:(h + 1) * H].astype(jnp.bfloat16)

        def send_lead(sel, c):
            part = slice(c * group, (c + 1) * group)
            start_both_sides(lead_r[sel][part], lead_l[sel][part])

        ld_k[0].wait()
        cast_and_send(K_SEL, 0)

        @pl.when((my == 0) | (my == 2))
        def _():
            pl.semaphore_wait(barrier, 2)

        @pl.when((my == 1) | (my == 3))
        def _():
            pl.semaphore_wait(barrier, 1)

        send_lead(K_SEL, 0)

        @pl.when(my == 2)
        def _():
            signal(go_sem, left)
            signal(go_sem, right)

        for c in range(1, N_LOAD):
            ld_k[c].wait()
            cast_and_send(K_SEL, c)
            send_lead(K_SEL, c)
        for c in range(N_LOAD):
            ld_v[c].wait()
            cast_and_send(V_SEL, c)
            send_lead(V_SEL, c)
        start_both_sides(trail_r, trail_l)

        ld_q.wait()
        qT = (f32buf[0] * scale).astype(jnp.bfloat16)

        def scores(a, b, m, l):
            s1 = lax.dot_general(kbuf[a], qT, CONTRACT_ROWS,
                                 preferred_element_type=jnp.float32)
            s2 = lax.dot_general(kbuf[b], qT, CONTRACT_ROWS,
                                 preferred_element_type=jnp.float32)
            m_new = jnp.maximum(jnp.max(s1, axis=0, keepdims=True),
                                jnp.max(s2, axis=0, keepdims=True))
            alpha = None
            if m is not None:
                m_new = jnp.maximum(m, m_new)
                alpha = jnp.exp2(m - m_new)
            p1 = jnp.exp2(s1 - m_new)
            p2 = jnp.exp2(s2 - m_new)
            l_blk = (jnp.sum(p1, axis=0, keepdims=True)
                     + jnp.sum(p2, axis=0, keepdims=True))
            l_new = l_blk if alpha is None else alpha * l + l_blk
            return (p1.astype(jnp.bfloat16), p2.astype(jnp.bfloat16), alpha), m_new, l_new

        def values(a, b, probs, acc):
            p1, p2, alpha = probs
            o = (jnp.dot(vbuf[a], p1, preferred_element_type=jnp.float32)
                 + jnp.dot(vbuf[b], p2, preferred_element_type=jnp.float32))
            return o if alpha is None else alpha * acc + o

        pair0 = ((OWN, 0), (OWN, 1))
        pair1 = ((FROM_LEFT, 0), (FROM_RIGHT, 1))
        pair2 = ((FROM_LEFT, 1), (FROM_RIGHT, 0))
        pair3 = ((DIAG, 0), (DIAG, 1))

        probs0, m, l = scores(*pair0, None, None)
        acc = values(*pair0, probs0, None)

        @pl.when(my == 1)
        def _():
            pl.semaphore_wait(go_sem, 1)
            start(lead_r[K_SEL] + lead_r[V_SEL] + trail_r)

        @pl.when(my == 3)
        def _():
            pl.semaphore_wait(go_sem, 1)
            start(lead_l[K_SEL] + lead_l[V_SEL] + trail_l)

        for sel in (K_SEL, V_SEL):
            for c in range(N_CHUNK):
                lead_r[sel][c].wait_recv()
                fwd_r[sel][c].start()
                lead_l[sel][c].wait_recv()
                fwd_l[sel][c].start()

        trail_r[K_SEL].wait_recv()
        trail_l[K_SEL].wait_recv()
        probs1, m, l = scores(*pair1, m, l)
        probs2, m, l = scores(*pair2, m, l)
        trail_r[V_SEL].wait_recv()
        trail_l[V_SEL].wait_recv()
        acc = values(*pair1, probs1, acc)
        acc = values(*pair2, probs2, acc)

        for sel in (K_SEL, V_SEL):
            for c in (lead_r[sel] + lead_l[sel] + fwd_r[sel] + fwd_l[sel]
                      + [trail_r[sel], trail_l[sel]]):
                c.wait_send()

        for c in fwd_r[K_SEL] + fwd_l[K_SEL]:
            c.wait_recv()
        probs3, m, l = scores(*pair3, m, l)
        for c in fwd_r[V_SEL] + fwd_l[V_SEL]:
            c.wait_recv()
        acc = values(*pair3, probs3, acc)
        o_ref[...] = acc * (1.0 / l)

    out_t = pl.pallas_call(
        body,
        out_shape=jax.ShapeDtypeStruct((D, S), jnp.float32),
        in_specs=[pl.BlockSpec(memory_space=pltpu.HBM)] * 3,
        out_specs=pl.BlockSpec(memory_space=pltpu.VMEM),
        scratch_shapes=[
            pltpu.VMEM((3, D, S), jnp.float32),
            pltpu.VMEM((N_DEV, 2, D, H), jnp.bfloat16),
            pltpu.VMEM((N_DEV, 2, D, H), jnp.bfloat16),
            pltpu.SemaphoreType.DMA((1 + 2 * N_LOAD,)),
            pltpu.SemaphoreType.DMA((4, 2, 2 * N_CHUNK)),
            pltpu.SemaphoreType.DMA((3, 2, 2 * N_CHUNK)),
            pltpu.SemaphoreType.REGULAR,
        ],
        compiler_params=pltpu.CompilerParams(
            collective_id=0,
            disable_semaphore_checks=True,
        ),
    )(q.T, k.T, v.T)
    return out_t.T
```
